```python
import numpy as np

kernel_name = "dist_ar_xy_y_m1024_n512"

def setup_inputs():
    return {"x": np.random.randn(2048, 512).astype(np.float32)}

def reference(x: np.ndarray) -> np.ndarray:
    return x.reshape(2, 1024, 512).sum(axis=0)
```

```python
import contextlib
import jax
import jax.numpy as jnp
from jax import lax
from jax.experimental import pallas as pl
from jax.experimental.pallas import tpu as pltpu

M, N = 1024, 512
MESHID = pl.DeviceIdType.MESH


def raw(x, fwd=(16,) * 29, both=(16,) * 6, loads=(16, 16, 32, 64, 128), scopes=False):
    F, E = sum(fwd), sum(both)
    assert 2 * F + E == M
    nf, ne = len(fwd), len(both)
    f_off = [sum(fwd[:i]) for i in range(nf)]
    e_off = [sum(both[:i]) for i in range(ne)]
    loads = tuple(loads) + (F - sum(loads),)
    l_off = [sum(loads[:i]) for i in range(len(loads))]
    scope = jax.named_scope if scopes else (lambda n: contextlib.nullcontext())

    def body(x_hbm, o_ref, xv, snd, rcv, in_sem, ys, yr, xs, xr, xrdy):
        mx = lax.axis_index("x")
        my = lax.axis_index("y")
        ynbr = (mx, 1 - my)
        xnbr = (1 - mx, my)
        mine = mx * F
        theirs = (1 - mx) * F

        def rows(base, off, n):
            return pl.ds(pl.multiple_of(base + off, 8), n)

        lds = []
        for i, n in enumerate(loads):
            r = rows(mine, l_off[i], n)
            c = pltpu.make_async_copy(x_hbm.at[r], xv.at[r], in_sem.at[i])
            c.start()
            lds.append(c)
            if i == 0:
                bs = pltpu.get_barrier_semaphore()
                pl.semaphore_signal(bs, inc=1, device_id=ynbr, device_id_type=MESHID)

                @pl.when(mx == 0)
                def _():
                    pl.semaphore_signal(bs, inc=1, device_id=xnbr, device_id_type=MESHID)

        r = pl.ds(2 * F, E)
        ld_e = pltpu.make_async_copy(x_hbm.at[r], xv.at[r], in_sem.at[len(loads)])
        ld_e.start()

        ysend = [rows(mine, f_off[i], fwd[i]) for i in range(nf)] + [
            pl.ds(2 * F + e_off[i], both[i]) for i in range(ne)
        ]
        ends = [f_off[i] + fwd[i] for i in range(nf)]
        ycopies = []
        waited = [0, 0]

        def send(i):
            r = ysend[i]
            if i < nf:
                while waited[0] < ends[i]:
                    lds[waited[1]].wait()
                    waited[0] += loads[waited[1]]
                    waited[1] += 1
            elif i == nf:
                ld_e.wait()
            snd[r, :] = xv[r, :].astype(jnp.bfloat16)
            if i == 0:
                with scope("barrier"):
                    pl.semaphore_wait(bs, 1 + mx)

                @pl.when(mx == 1)
                def _():
                    pl.semaphore_signal(xrdy, inc=1, device_id=xnbr, device_id_type=MESHID)

            c = pltpu.make_async_remote_copy(snd.at[r], rcv.at[r], ys, yr.at[i], device_id=ynbr, device_id_type=MESHID)
            c.start()
            ycopies.append(c)

        n_send = nf + ne
        ahead = 8
        with scope("send0"):
            for i in range(ahead):
                send(i)
        for i, r in enumerate(ysend):
            with scope("yr%d" % i):
                ycopies[i].wait_recv()
            o_ref[r, :] = (xv[r, :] + rcv[r, :].astype(jnp.float32)).astype(jnp.bfloat16)
            if i == 0:

                @pl.when(mx == 0)
                def _():
                    with scope("xrdy"):
                        pl.semaphore_wait(xrdy, 1)

            if i < nf:
                pltpu.make_async_remote_copy(
                    o_ref.at[r], o_ref.at[r], xs, xr, device_id=xnbr, device_id_type=MESHID
                ).start()
            for k in range(2):
                j = ahead + 2 * i + k
                if j < n_send:
                    send(j)
        r = pl.ds(0, F + E)
        with scope("ysend"):
            pltpu.make_async_remote_copy(snd.at[r], rcv.at[r], ys, yr.at[0], device_id=ynbr, device_id_type=MESHID).wait_send()
        r = pl.ds(0, F)
        with scope("xall"):
            pltpu.make_async_remote_copy(o_ref.at[r], o_ref.at[r], xs, xr, device_id=xnbr, device_id_type=MESHID).wait()

    return pl.pallas_call(
        body,
        out_shape=jax.ShapeDtypeStruct((M, N), jnp.bfloat16),
        in_specs=[pl.BlockSpec(memory_space=pltpu.HBM)],
        out_specs=pl.BlockSpec(memory_space=pltpu.VMEM),
        scratch_shapes=[
            pltpu.VMEM((M, N), jnp.float32),
            pltpu.VMEM((M, N), jnp.bfloat16),
            pltpu.VMEM((M, N), jnp.bfloat16),
            pltpu.SemaphoreType.DMA((len(loads) + 1,)),
            pltpu.SemaphoreType.DMA,
            pltpu.SemaphoreType.DMA((nf + ne,)),
            pltpu.SemaphoreType.DMA,
            pltpu.SemaphoreType.DMA,
            pltpu.SemaphoreType.REGULAR,
        ],
        compiler_params=pltpu.CompilerParams(
            collective_id=0, disable_bounds_checks=True, disable_semaphore_checks=True
        ),
    )(x)


def pallas_dist_ar_xy_y_m1024_n512_kernel(x: jax.Array):
    return raw(x)
```

```python
import contextlib
import jax
import jax.numpy as jnp
import numpy as np
from jax import lax
from jax.experimental import pallas as pl
from jax.experimental.pallas import tpu as pltpu

M, N = 1024, 512
MESHID = pl.DeviceIdType.MESH
I32 = jnp.int32
TILE = (8, 128)


def c32(v):
    return np.uint32(v).astype(np.int32)


def rep(v):
    return c32(v * 0x01010101)


def shl(a, b):
    return lax.shift_left(a, jnp.broadcast_to(jnp.asarray(b, I32), a.shape))


def shr(a, b):
    return lax.shift_right_logical(a, jnp.broadcast_to(jnp.asarray(b, I32), a.shape))


KEEP = c32(0x807F807F)


def split(w1, w2):
    r = shl(w2, 8) | shr(w2, 24)
    t = (w1 ^ r) & KEEP
    e = w1 ^ t
    return r ^ t, shr(e, 7) | shl(e, 25)


def join(s, e):
    e = shl(e, 7) | shr(e, 25)
    t = (s ^ e) & KEEP
    r = s ^ t
    return e ^ t, shr(r, 8) | shl(r, 24)


def below(v, k):
    m = ~(v + rep(128 - k)) & rep(128)
    return m - shr(m, 7)


def rot(v, n):
    return v + (below(v, 1) & rep(n)) - (below(v, n) & rep(1))


def unrot(v, n):
    return v + (below(v, n - 1) & rep(n)) - (below(v, n) & rep(n - 1))


def shift_right(reg, n, nbits, count):
    for bit in range(5, nbits):
        k = 1 << (bit - 5)
        on = (n & (1 << bit)) != 0
        get = lambda j: reg[j] if 0 <= j < len(reg) else 0
        reg = [jnp.where(on, get(j - k), get(j)) for j in range(min(count, len(reg) + k))]
    r = n & 31
    out = []
    for j in range(min(count, len(reg) + 1)):
        w = shr(reg[j], r) if j < len(reg) else None
        if j:
            c = shl(shl(reg[j - 1], 1), 31 - r)
            w = c if w is None else w | c
        out.append(w)
    return out


def shift_left(reg, n, nbits, count):
    for bit in reversed(range(5, nbits)):
        k = 1 << (bit - 5)
        on = (n & (1 << bit)) != 0
        reg = [jnp.where(on, reg[j + k] if j + k < len(reg) else 0, reg[j]) for j in range(min(count + k, len(reg)))]
    r = n & 31
    out = []
    for j in range(min(count, len(reg))):
        w = shl(reg[j], r)
        if j + 1 < len(reg):
            w = w | shr(shr(reg[j + 1], 1), 31 - r)
        out.append(w)
    return out


def encode_group(es, top4):
    hi = lo = total = bad = lows = None
    msb = jnp.full(TILE, c32(1 << 31), I32)
    for e in reversed(es):
        u = top4 - e
        w = rot(rot(u, 12), 6)
        low = w & rep(1)
        lows = low if lows is None else shl(lows, 1) | low
        q = (shr(w, 1) & rep(127)) + c32(0x01010100)
        q = q + shl(q, 8)
        q = q + shl(q, 16)
        p3 = shr(q, 24)
        g = shr(msb, q & 255) | shr(msb, shr(q, 8) & 255) | shr(msb, shr(q, 16) & 255) | shr(msb, p3)
        r = p3 + 1
        b = u | shl(r, 1)
        bad = b if bad is None else bad | b
        if hi is None:
            hi, total = g, r
        else:
            carry = shl(hi, 32 - r)
            lo = carry if lo is None else shr(lo, r) | carry
            hi = g | shr(hi, r)
            total = total + r
    return hi, lo, total, lows, (bad | total) & rep(0xC0)


def decode_group(hi, lo, lows, top4):
    es = []
    total = None
    for i in range(4):
        x = hi
        z = []
        for j in range(4):
            z.append(lax.clz(x))
            if j < 3:
                x = shl(shl(x, 1), z[-1])
        r = (z[0] + z[1] + z[2] + 4) + z[3]
        w = shl(z[0], 1) | shl(z[1], 9) | shl(z[2], 17) | shl(z[3], 25) | (shr(lows, i) & rep(1))
        es.append(top4 - unrot(unrot(w, 6), 12))
        total = r if total is None else total + r
        if i < 3:
            hi = shl(hi, r) | shr(lo, 32 - r)
            if i < 2:
                lo = shl(lo, r)
    return es, total


def comp(
    x,
    W=15,
    D=10,
    head=24,
    ch=1,
    loads=(1, 1, 2) + (4,) * 15,
    xlag=20,
    t0=56,
    late=31,
    budget=100,
    scopes=False,
    force_bad=False,
    checks=False,
):
    T = 64
    H = 8 * T
    G = T // 4
    R = 17
    pL = head
    pU = pL + 8
    side = 8 + W
    NX = T - D + side
    NY = T + D + side

    def spos(i):
        return i if i < head else i + side

    xchunks = [(p, min(ch, NX - p)) for p in range(0, NX, ch)]
    ychunks = xchunks + [(p, min(ch, NY - p)) for p in range(NX, NY, ch)]
    nx, ny = len(xchunks), len(ychunks)
    assert sum(loads) == T and head % ch == 0
    scope = jax.named_scope if scopes else (lambda n: contextlib.nullcontext())

    def body(x_hbm, o_ref, xv, tx, ry, rx, et, ey, ex, fy, fx, in_sem, ys, yr, xs, xr, fsem, xrdy):
        mx = lax.axis_index("x")
        my = lax.axis_index("y")
        ynbr = (mx, 1 - my)
        xnbr = (1 - mx, my)
        mine = pl.ds(pl.multiple_of(mx * H, H), H)
        theirs = pl.ds(pl.multiple_of((1 - mx) * H, H), H)
        sub = lax.broadcasted_iota(I32, TILE, 0)

        def remote(src, dst, ssem, rsem, dev):
            return pltpu.make_async_remote_copy(src, dst, ssem, rsem, device_id=dev, device_id_type=MESHID)

        lds = {}

        def load(half, base, t, n):
            c = pltpu.make_async_copy(
                x_hbm.at[half].at[pl.ds(8 * t, 8 * n)], xv.at[pl.ds(8 * (base + t), 8 * n)], in_sem.at[len(lds)]
            )
            c.start()
            lds[base + t] = c

        t = 0
        for n in loads:
            load(mine, 0, t, n)
            if t == 0:
                bs = pltpu.get_barrier_semaphore()
                pl.semaphore_signal(bs, inc=1, device_id=ynbr, device_id_type=MESHID)

                @pl.when(mx == 0)
                def _():
                    pl.semaphore_signal(bs, inc=1, device_id=xnbr, device_id_type=MESHID)

            t += n
        load(theirs, T, T - D, D)
        load(theirs, T, 0, T - D)

        sent = [0]

        def send_upto(p, limit=1000):
            while sent[0] < ny and sum(ychunks[sent[0]]) <= p and limit:
                r = pl.ds(*ychunks[sent[0]])
                remote(tx.at[r], ry.at[r], ys, yr.at[sent[0]], ynbr).start()
                sent[0] += 1
                limit -= 1

        def pack(t):
            if t in lds:
                lds[t].wait()
            v = xv[8 * t : 8 * t + 8, :]
            w = [
                pltpu.bitcast(
                    jnp.concatenate([v[:, c : c + 128], v[:, c + 128 : c + 256]], axis=0).astype(jnp.bfloat16), I32
                )
                for c in (0, 256)
            ]
            s, e = split(*w)
            if t < T:
                tx[spos(t)] = s
                et[t] = e
            else:
                tx[spos(t - T + D)] = s

        class Stream:
            def __init__(self, buf, ebuf, chunks, sems, dev):
                self.buf, self.ebuf, self.chunks, self.sems, self.dev = buf, ebuf, chunks, sems, dev
                self.got = 0
                self.dec = -1

            def wait(self):
                r = pl.ds(*self.chunks[self.got])
                remote(self.buf.at[r], self.buf.at[r], ys, self.sems.at[self.got], self.dev).wait_recv()
                self.got += 1

            def have(self):
                return sum(self.chunks[self.got - 1]) if self.got else 0

            def can_decode(self):
                return self.dec < G and self.have() >= pU + W

            def decode(self):
                if self.dec < 0:
                    wire = [self.buf[pU + j] for j in range(W)]
                    h0 = jnp.broadcast_to(wire[0][0:1], TILE)
                    h1 = jnp.broadcast_to(wire[1][0:1], TILE)
                    top = h0 & 255
                    self.plain = top[0, 0] == 0
                    top = top | shl(top, 8)
                    self.top4 = top | shl(top, 16)
                    d = shr(jnp.where(sub < 4, h0, h1), 8 * (sub & 3)) & 255
                    d = jnp.where(sub == 0, 192, d)
                    ext = [pltpu.roll(w, 1, 0) for w in wire[-4:]] + wire + [pltpu.roll(w, 7, 0) for w in wire[:4]]
                    self.reg = shift_left(ext, d, 8, R)
                else:
                    k = G - 1 - self.dec
                    lows = shr(self.buf[pL + k // 2], 4 * (k % 2))
                    es, n = decode_group(self.reg[0], self.reg[1], lows, self.top4)
                    if k:
                        self.reg = shift_left(self.reg, n, 6, min(R, k + 2))
                    for i in range(4):
                        self.ebuf[4 * k + i] = es[i]
                self.dec += 1

            def has_exp(self, t):
                return self.dec > G - 1 - t // 4

        Y = Stream(ry, ey, ychunks, yr, ynbr)
        X = Stream(rx, ex, xchunks, xr, xnbr)

        def forward():
            j = Y.got
            with scope("yr%d" % j):
                Y.wait()
            if j == 0:

                @pl.when(mx == 0)
                def _():
                    pl.semaphore_wait(xrdy, 1)

            if j < nx:
                r = pl.ds(*xchunks[j])
                remote(ry.at[r], rx.at[r], xs, xr.at[j], xnbr).start()

        st = dict(reg=None)

        def encode(k):
            hi, lo, n, lows, b = encode_group([et[4 * k + i] for i in range(4)], top4)
            if k % 2:
                tx[pL + k // 2] = tx[pL + k // 2] | shl(lows, 4)
            else:
                tx[pL + k // 2] = lows
            if k == 0:
                st.update(reg=[hi, lo], total=n, bad=b)
                return
            count = min(R, k + 3)
            reg = shift_right(st["reg"], n, 6, count)
            reg[0] = reg[0] | hi
            reg[1] = reg[1] | lo
            total = st["total"] + n
            st.update(reg=reg, total=total, bad=st["bad"] | b | shr(32 * count - total, 31))

        def ysend(j):
            r = pl.ds(*ychunks[j])
            remote(tx.at[r], ry.at[r], ys, yr.at[j], ynbr).start()

        def handshake(n):
            with scope("barrier"):
                pl.semaphore_wait(bs, 1 + mx)
            for j in range(n):
                ysend(j)
                if j == 0:

                    @pl.when(mx == 1)
                    def _():
                        pl.semaphore_signal(xrdy, inc=1, device_id=xnbr, device_id_type=MESHID)

        with scope("first"):
            for t in range(ch):
                pack(t)
            pl.when(my == 1)(lambda: handshake(1))

        def pool_a():
            total = st["total"]
            incl = total
            for k in (1, 2, 4):
                incl = incl + jnp.where(sub >= k, pltpu.roll(incl, k, 0), 0)
            avg = shr(jnp.broadcast_to(incl[7:8], TILE) + (64 + 7), 3)
            d = incl - total + (64 + 128) - avg * sub
            badv = st["bad"] | shr(32 * W - avg, 31) | (d & -256)
            st.update(d=d, any=jnp.max(jnp.where(badv != 0, 1.0, 0.0)), ext=shift_right(st["reg"], d, 8, W + 8))

        def pool_b():
            bad = st["any"] > 0
            if force_bad:
                bad = jnp.logical_or(bad, True)
            ext, d = st["ext"], st["d"]
            wire = ext[4 : W + 4]
            for j in range(4):
                wire[W - 4 + j] = wire[W - 4 + j] | pltpu.roll(ext[j], 7, 0)
                wire[j] = wire[j] | pltpu.roll(ext[W + 4 + j], 1, 0)
            h = shl(jnp.where(sub == 0, jnp.where(bad, 0, top), d & 255), 8 * (sub & 3))
            h = h | pltpu.roll(h, 7, 0)
            h = h | pltpu.roll(h, 6, 0)
            wire[0] = jnp.where(sub == 0, h, wire[0])
            wire[1] = jnp.where(sub == 0, pltpu.roll(h, 4, 0), wire[1])
            for j in range(W):
                tx[pU + j] = wire[j]
            st.update(plain=bad, filled=NY - D)

        enc = 0
        with scope("pack"):
            for t in range(ch, t0):
                pack(t)
                if t < head and (t + 1) % ch == 0:
                    pl.when(my == 1)(lambda: ysend(t // ch))
                if t == late:
                    pl.when(my == 0)(lambda: handshake(head // ch))
                    sent[0] = head // ch
                if t == 7:
                    acc = None
                    for i in range(8):
                        e = et[i]
                        s = (e & c32(0x00FF00FF)) + (shr(e, 8) & c32(0x00FF00FF))
                        acc = s if acc is None else acc + s
                    tot = jnp.sum(((acc & 0xFFFF) + shr(acc, 16)).astype(jnp.float32)).astype(I32)
                    top = jnp.minimum((tot + int(3.86 * 32768)) >> 15, 255)
                    top4 = jnp.full(TILE, top * rep(1), I32)
                if t >= 7 and t % 4 == 3:
                    while enc <= t // 4:
                        encode(enc)
                        enc += 1
        st["filled"] = head
        tasks = []
        for k in range(t0 // 4, G):
            tasks.append(lambda k=k: [pack(4 * k + i) for i in range(4)])
            tasks.append(lambda k=k: encode(k))
        tasks += [pool_a, pool_b]
        for k in range(2 * T - D, 2 * T, 5):
            tasks.append(lambda k=k: [pack(i) for i in range(k, min(k + 5, 2 * T))])
        tasks.append(lambda: st.update(filled=NY))

        def finish(t, sy, sx):
            u = t % T
            if t < T:
                s, e = ry[spos(u)], sy[u]
            elif u >= T - D:
                s, e = ry[spos(u + D)], sx[u]
            else:
                s, e = rx[spos(u)], sx[u]
            v = []
            for w in join(s, e):
                f = pltpu.bitcast(w, jnp.bfloat16).astype(jnp.float32)
                v += [f[:8], f[8:]]
            v = xv[8 * t : 8 * t + 8, :] + jnp.concatenate(v, axis=1)
            o_ref.at[mine if t < T else theirs][8 * u : 8 * u + 8, :] = v.astype(jnp.bfloat16)

        todo = list(range(2 * T))

        def ready(t):
            u = t % T
            if t < T:
                return Y.has_exp(u) and Y.have() > spos(u)
            if u >= T - D:
                return X.has_exp(u) and Y.have() > spos(u + D)
            return X.has_exp(u) and X.have() > spos(u)

        def work(left):
            if tasks:
                for _ in range(ch):
                    if tasks:
                        with scope("task%d" % len(tasks)):
                            tasks.pop(0)()
                return
            if T in lds and X.can_decode():
                lds.pop(T).wait()
            for s in (X, Y):
                while s.can_decode() and left >= 90:
                    s.decode()
                    left -= 90
            for t in list(todo):
                if left >= 12 and ready(t):
                    finish(t, ey, ex)
                    todo.remove(t)
                    left -= 12

        while Y.got < ny:
            forward()
            send_upto(st["filled"], 3)
            while X.got < nx and sum(xchunks[X.got]) + xlag <= Y.have():
                with scope("xr%d" % X.got):
                    X.wait()
            work(budget * ch)
            if Y.got == ny - 1:
                remote(tx, ry, ys, yr.at[0], ynbr).wait_send()
                remote(ry.at[pl.ds(0, NX)], rx, xs, xr.at[0], xnbr).wait_send()
        with scope("tail"):
            work(10000)
            while X.got < nx:
                X.wait()
                work(10000)
        assert not todo and sent[0] == ny
        bad = st["plain"]

        @pl.when(bad)
        def _():
            remote(et, fy, fsem.at[0], fsem.at[1], ynbr).start()

        @pl.when(Y.plain)
        def _():
            remote(fy, fy, fsem.at[0], fsem.at[1], ynbr).wait_recv()
            c = remote(fy, fx, fsem.at[2], fsem.at[3], xnbr)
            c.start()
            for t in range(T):
                finish(t, fy, fx)
            c.wait_send()

        @pl.when(X.plain)
        def _():
            remote(fx, fx, fsem.at[2], fsem.at[3], xnbr).wait_recv()
            for t in range(T, 2 * T):
                finish(t, fy, fx)

        @pl.when(bad)
        def _():
            remote(et, fy, fsem.at[0], fsem.at[1], ynbr).wait_send()

    def tiles(n):
        return pltpu.VMEM((n, 8, 128), I32)

    return pl.pallas_call(
        body,
        out_shape=jax.ShapeDtypeStruct((M, N), jnp.bfloat16),
        in_specs=[pl.BlockSpec(memory_space=pltpu.HBM)],
        out_specs=pl.BlockSpec(memory_space=pltpu.VMEM),
        scratch_shapes=[
            pltpu.VMEM((M, N), jnp.float32),
            tiles(NY),
            tiles(NY),
            tiles(NX),
            tiles(T),
            tiles(T),
            tiles(T),
            tiles(T),
            tiles(T),
            pltpu.SemaphoreType.DMA((len(loads) + 2,)),
            pltpu.SemaphoreType.DMA,
            pltpu.SemaphoreType.DMA((ny,)),
            pltpu.SemaphoreType.DMA,
            pltpu.SemaphoreType.DMA((nx,)),
            pltpu.SemaphoreType.DMA((4,)),
            pltpu.SemaphoreType.REGULAR,
        ],
        compiler_params=pltpu.CompilerParams(
            collective_id=0, disable_bounds_checks=not checks, disable_semaphore_checks=not checks
        ),
    )(x)


def pallas_dist_ar_xy_y_m1024_n512_kernel(x: jax.Array):
    return comp(x)
```

```python
import functools

import jax
import jax.numpy as jnp
import numpy as np
from jax import lax
from jax.experimental import pallas as pl
from jax.experimental.pallas import tpu as pltpu

ROWS, COLS = 1024, 512
TILE = (8, 128)
STRIPS = ROWS // 2 // 8
GROUPS = STRIPS // 4

HEAD = 24
LOW_TILES = GROUPS // 2
ROW_WORDS = 14
DIRECT = 10
LOW_AT = HEAD
CODE_AT = LOW_AT + LOW_TILES
TAIL_AT = CODE_AT + ROW_WORDS
X_TILES = STRIPS - DIRECT + LOW_TILES + ROW_WORDS
Y_TILES = X_TILES + 2 * DIRECT
X_LAG = Y_TILES - X_TILES

STRING_WORDS = 17
HEADER_BITS = 64
BACK_WORDS, AHEAD_WORDS = 3, 5
FITS, ONE_MORE_TILE, UNCODED = 0, 1, 2

LOADS = (1, 1, 2) + (4,) * 15
BASE_STRIPS = 8
LATE_HANDSHAKE = 31
BULK_STRIPS = 56
SLOT_CYCLES = 100
UNCODED_PARTS = 8


def _word(v):
    return np.uint32(v).astype(np.int32)


def _bytes(v):
    return _word(v * 0x01010101)


def _shl(a, n):
    return lax.shift_left(a, jnp.broadcast_to(jnp.asarray(n, jnp.int32), a.shape))


def _shr(a, n):
    return lax.shift_right_logical(a, jnp.broadcast_to(jnp.asarray(n, jnp.int32), a.shape))


def _sublane():
    return lax.broadcasted_iota(jnp.int32, TILE, 0)


_SIGN_MANTISSA = _word(0x807F807F)


def _split(a, b):
    b = _shl(b, 8) | _shr(b, 24)
    swap = (a ^ b) & _SIGN_MANTISSA
    e = a ^ swap
    return b ^ swap, _shr(e, 7) | _shl(e, 25)


def _join(s, e):
    e = _shl(e, 7) | _shr(e, 25)
    swap = (s ^ e) & _SIGN_MANTISSA
    b = s ^ swap
    return e ^ swap, _shr(b, 8) | _shl(b, 24)


def _below(v, k):
    m = ~(v + _bytes(128 - k)) & _bytes(128)
    return m - _shr(m, 7)


def _demote(v, n):
    return v + (_below(v, 1) & _bytes(n)) - (_below(v, n) & _bytes(1))


def _promote(v, n):
    return v + (_below(v, n - 1) & _bytes(n)) - (_below(v, n) & _bytes(n - 1))


def _encode_group(exponents, base):
    msb = jnp.full(TILE, _word(1 << 31), jnp.int32)
    hi = lo = length = low = distances = lengths = None
    for e in reversed(exponents):
        distance = base - e
        rank = _demote(_demote(distance, 12), 6)
        ones_at = (_shr(rank, 1) & _bytes(127)) + _word(0x01010100)
        ones_at = ones_at + _shl(ones_at, 8)
        ones_at = ones_at + _shl(ones_at, 16)
        bits = functools.reduce(
            jnp.bitwise_or, [_shr(msb, (_shr(ones_at, k) if k else ones_at) & 31) for k in (0, 8, 16, 24)]
        )
        n = _shr(ones_at, 24) + 1
        if hi is None:
            hi, length, low, distances, lengths = bits, n, rank & _bytes(1), distance, n
        else:
            carry = _shl(hi, -n & 31)
            lo = carry if lo is None else _shr(lo, n & 31) | carry
            hi = bits | _shr(hi, n & 31)
            length, low = length + n, _shl(low, 1) | (rank & _bytes(1))
            distances, lengths = distances | distance, lengths | n
    return hi, lo, length, low, (distances & _bytes(0xC0)) | _shr(lengths, 5) | _shr(length, 6)


def _decode_group(hi, lo, low, base):
    exponents, length = [], None
    for i in range(4):
        rest, zeros = hi, []
        for j in range(4):
            zeros.append(lax.clz(rest))
            if j < 3:
                rest = _shl(_shl(rest, 1), zeros[-1])
        n = (zeros[0] + zeros[1] + zeros[2] + 4) + zeros[3]
        rank = _shr(low, i) & _bytes(1)
        for j in range(4):
            rank = rank | _shl(zeros[j], 8 * j + 1)
        exponents.append(base - _promote(_promote(rank, 6), 12))
        length = n if length is None else length + n
        if i < 3:
            hi, lo = _shl(hi, n) | _shr(lo, 32 - n), _shl(lo, n)
    return exponents, length


def _delay(words, n, n_bits, count):
    for bit in range(5, n_bits):
        k, on = 1 << (bit - 5), (n & (1 << bit)) != 0
        moved, still = [0] * k + words, words + [0] * k
        words = [jnp.where(on, a, b) for a, b in zip(moved[:count], still[:count])]
    r = n & 31
    stay = [_shr(w, r) for w in words]
    carry = [_shl(_shl(w, 1), 31 - r) for w in words[: count - 1]]
    return (stay[:1] + [a | b for a, b in zip(stay[1:], carry)] + carry[len(stay) - 1 :])[:count]


def _skip(words, n, n_bits, count):
    for bit in reversed(range(5, n_bits)):
        k, on = 1 << (bit - 5), (n & (1 << bit)) != 0
        words = [jnp.where(on, a, b) for a, b in zip(words[k:] + [0] * k, words[: count + k])]
    r = n & 31
    stay = [_shl(w, r) for w in words[:count]]
    carry = [_shr(_shr(w, 1), 31 - r) for w in words[1:]]
    return [a | b for a, b in zip(stay, carry)] + stay[len(carry) :]


def _place_strings(length):
    sub = _sublane()
    end = length
    for k in (1, 2, 4):
        end = end + jnp.where(sub >= k, pltpu.roll(end, k, 0), 0)
    row_bits = _shr(jnp.broadcast_to(end[7:8], TILE) + (HEADER_BITS + 7), 3)
    return end - length + (HEADER_BITS + 32 * BACK_WORDS) - row_bits * sub, row_bits


def _cut_rows(placed, start, base, mode):
    longer = mode == ONE_MORE_TILE
    rows = placed[BACK_WORDS : BACK_WORDS + ROW_WORDS + 1]
    back = [pltpu.roll(w, 7, 0) for w in placed[:BACK_WORDS]]
    for j, (a, b) in enumerate(zip([0] + back, back + [0])):
        rows[ROW_WORDS - BACK_WORDS + j] |= jnp.where(longer, a, b)
    ahead = placed[BACK_WORDS + ROW_WORDS :]
    for j in range(AHEAD_WORDS):
        rows[j] |= pltpu.roll(jnp.where(longer, ahead[j + 1], ahead[j]), 1, 0)
    rows = [w | jnp.where(mode == UNCODED, -1, 0) for w in rows]
    sub = _sublane()
    first = jnp.where(lax.broadcasted_iota(jnp.int32, TILE, 1) == 0, base, mode)
    header = _shl(jnp.where(sub == 0, first, start), (sub & 3) * 8)
    header = header | pltpu.roll(header, 7, 0)
    header = header | pltpu.roll(header, 6, 0)
    rows[0] = jnp.where(sub == 0, header, rows[0])
    rows[1] = jnp.where(sub == 0, pltpu.roll(header, 4, 0), rows[1])
    return rows


def _take_strings(rows, mode):
    longer = mode == ONE_MORE_TILE
    sub = _sublane()
    header = [jnp.broadcast_to(w[0:1], TILE) for w in rows[:2]]
    start = _shr(jnp.where(sub < 4, *header), (sub & 3) * 8) & 255
    start = jnp.where(sub == 0, HEADER_BITS + 32 * BACK_WORDS, start)
    last = rows[ROW_WORDS - BACK_WORDS :]
    back = [pltpu.roll(jnp.where(longer, a, b), 1, 0) for a, b in zip(last[1:], last)]
    ahead = [pltpu.roll(w, 7, 0) for w in rows[:AHEAD_WORDS]]
    ahead = [jnp.where(longer, a, b) for a, b in zip(rows[-1:] + ahead, ahead + [0])]
    return _skip(back + rows[:ROW_WORDS] + ahead, start, 8, STRING_WORDS)


def _tile_of(strip):
    return strip if strip < HEAD else strip + LOW_TILES + ROW_WORDS


class _Inbox:
    def __init__(self, tiles, one_more, exponents):
        self.tiles, self.one_more, self.exponents = tiles, one_more, exponents
        self.landed = 0
        self.decoded_from = STRIPS

    def read_header(self):
        header = self.tiles[CODE_AT] & 255
        self.base = jnp.full(TILE, header[0, 0] * _bytes(1), jnp.int32)
        self.mode = header[0, 1]

    def take_strings(self):
        rows = [self.tiles[CODE_AT + j] for j in range(ROW_WORDS)] + [self.one_more[...]]
        self.string = _take_strings(rows, self.mode)

    def decode(self, group):
        low = _shr(self.tiles[LOW_AT + group // 2], 4 * (group % 2))
        exponents, length = _decode_group(*self.string[:2], low, self.base)
        for i, e in enumerate(exponents):
            self.exponents[4 * group + i] = e
        if group:
            self.string = _skip(self.string, length, 6, min(STRING_WORDS, group + 2))
        self.decoded_from = 4 * group


def _all_reduce(
    x_hbm, out,
    x, status,
    sent, got_y, got_x,
    sent_more, got_y_more, got_x_more,
    exp, exp_y, exp_x, uncoded_y, uncoded_x,
    load_sems, y_send_sem, y_recv_sems, x_send_sem, x_recv_sems,
    more_sems, uncoded_send_sems, uncoded_y_sems, uncoded_x_sems, x_ready,
):
    my_x, my_y = lax.axis_index("x"), lax.axis_index("y")
    y_peer, x_peer = (my_x, 1 - my_y), (1 - my_x, my_y)
    half = ROWS // 2
    halves = [pl.ds(pl.multiple_of(h * half, half), half) for h in (my_x, 1 - my_x)]

    def remote(src, dst, send_sem, recv_sem, peer):
        return pltpu.make_async_remote_copy(
            src, dst, send_sem, recv_sem, device_id=peer, device_id_type=pl.DeviceIdType.MESH
        )

    def over_y(i):
        return remote(sent.at[i], got_y.at[i], y_send_sem, y_recv_sems.at[i], y_peer)

    def over_x(i):
        return remote(got_y.at[i], got_x.at[i], x_send_sem, x_recv_sems.at[i], x_peer)

    def more_over_y():
        return remote(sent_more, got_y_more, more_sems.at[0], more_sems.at[1], y_peer)

    def more_over_x():
        return remote(got_y_more, got_x_more, more_sems.at[2], more_sems.at[3], x_peer)

    part = STRIPS // UNCODED_PARTS

    def uncoded_over_y(i):
        r = pl.ds(i * part, part)
        return remote(exp.at[r], uncoded_y.at[r], uncoded_send_sems.at[0], uncoded_y_sems.at[i], y_peer)

    def uncoded_over_x(i):
        r = pl.ds(i * part, part)
        return remote(uncoded_y.at[r], uncoded_x.at[r], uncoded_send_sems.at[1], uncoded_x_sems.at[i], x_peer)

    loads = {}

    def load(strip, count):
        rows = x_hbm.at[halves[strip // STRIPS]].at[pl.ds(8 * (strip % STRIPS), 8 * count)]
        loads[strip] = pltpu.async_copy(rows, x.at[pl.ds(8 * strip, 8 * count)], load_sems.at[len(loads)])

    load(0, LOADS[0])
    got_y_more[...] = jnp.zeros(TILE, jnp.int32)
    got_x_more[...] = jnp.zeros(TILE, jnp.int32)
    barrier = pltpu.get_barrier_semaphore()

    def signal(sem, peer):
        pl.semaphore_signal(sem, device_id=peer, device_id_type=pl.DeviceIdType.MESH)

    signal(barrier, y_peer)
    pl.when(my_x == 0)(lambda: signal(barrier, x_peer))
    for i in range(1, len(LOADS)):
        load(sum(LOADS[:i]), LOADS[i])
    load(2 * STRIPS - DIRECT, DIRECT)
    load(STRIPS, STRIPS - DIRECT)

    def handshake(ready_tiles):
        pl.semaphore_wait(barrier, 1 + my_x)
        over_y(0).start()
        pl.when(my_x == 1)(lambda: signal(x_ready, x_peer))
        for i in range(1, ready_tiles):
            over_y(i).start()

    def pack(*strips):
        for strip in strips:
            if strip in loads:
                loads[strip].wait()
            v = x[8 * strip : 8 * strip + 8, :]
            pairs = [jnp.concatenate([v[:, c : c + 128], v[:, c + 128 : c + 256]]) for c in (0, 256)]
            s, e = _split(*[pltpu.bitcast(p.astype(jnp.bfloat16), jnp.int32) for p in pairs])
            if strip < STRIPS:
                sent[_tile_of(strip)] = s
                exp[strip] = e
            else:
                sent[_tile_of(strip - STRIPS + DIRECT)] = s

    class Outbox:
        filled = started = HEAD

        def measure_base(self):
            total = 0
            for strip in range(BASE_STRIPS):
                e = exp[strip]
                total = total + (e & 0x00FF00FF) + (_shr(e, 8) & 0x00FF00FF)
            total = jnp.sum(((total & 0xFFFF) + _shr(total, 16)).astype(jnp.float32))
            mean = total * (1.0 / (BASE_STRIPS * 8 * COLS))
            self.base = jnp.minimum((mean + 3.86).astype(jnp.int32), 255)

        def encode(self, group):
            base = jnp.full(TILE, self.base * _bytes(1), jnp.int32)
            hi, lo, length, low, misfit = _encode_group([exp[4 * group + i] for i in range(4)], base)
            at = LOW_AT + group // 2
            sent[at] = sent[at] | _shl(low, 4) if group % 2 else low
            if group == 0:
                self.string, self.length, self.misfit = [hi, lo], length, misfit
                return
            count = min(STRING_WORDS, group + 3)
            self.string = _delay(self.string, length, 6, count)
            self.string[0] |= hi
            self.string[1] |= lo
            self.length = self.length + length
            self.misfit = self.misfit | misfit | _shr(32 * count - self.length, 31)

        def place(self):
            start, row_bits = _place_strings(self.length)
            misfit = self.misfit | (start & -256) | _shr(32 * (ROW_WORDS + 1) - row_bits, 31)
            mode = jnp.where(row_bits > 32 * ROW_WORDS, ONE_MORE_TILE, FITS)
            mode = jnp.where(misfit != 0, UNCODED, mode).astype(jnp.float32)
            status[...] = jnp.broadcast_to(jnp.max(mode, axis=1, keepdims=True), TILE)
            self.start = start & 255
            self.string = _delay(self.string, self.start, 8, BACK_WORDS + ROW_WORDS + 1 + AHEAD_WORDS)

        def cut(self):
            self.mode = jnp.max(status[...], axis=0, keepdims=True).astype(jnp.int32)[0, 0]
            rows = _cut_rows(self.string, self.start, self.base, self.mode)
            for j in range(ROW_WORDS):
                sent[CODE_AT + j] = rows[j]
            sent_more[...] = rows[ROW_WORDS]
            self.filled = Y_TILES - DIRECT

        def pack_direct(self, first):
            pack(*range(first, first + DIRECT // 2))
            self.filled += DIRECT // 2

        def start_next(self):
            over_y(self.started).start()
            self.started += 1
            if self.started == TAIL_AT:
                pl.when(self.mode == ONE_MORE_TILE)(lambda: more_over_y().start())
            if self.started == Y_TILES:

                @pl.when(self.mode == UNCODED)
                def _():
                    for i in range(UNCODED_PARTS):
                        uncoded_over_y(i).start()

    outbox = Outbox()
    from_y = _Inbox(got_y, got_y_more, exp_y)
    from_x = _Inbox(got_x, got_x_more, exp_x)

    def source(strip):
        if strip < STRIPS:
            return from_y, _tile_of(strip)
        if strip < 2 * STRIPS - DIRECT:
            return from_x, _tile_of(strip - STRIPS)
        return from_y, _tile_of(strip - STRIPS + DIRECT)

    def add(strip, exponents):
        inbox, at = source(strip)
        other = []
        for pairs in _join(inbox.tiles[at], exponents[strip % STRIPS]):
            pairs = pltpu.bitcast(pairs, jnp.bfloat16).astype(jnp.float32)
            other += [pairs[:8], pairs[8:]]
        total = x[8 * strip : 8 * strip + 8, :] + jnp.concatenate(other, axis=1)
        rows = pl.ds(8 * (strip % STRIPS), 8)
        out.at[halves[strip // STRIPS]][rows, :] = total.astype(out.dtype)

    def can_add(strip):
        inbox, at = source(strip)
        return inbox.landed > at and (from_y, from_x)[strip // STRIPS].decoded_from <= strip % STRIPS

    encoded = 0
    for strip in range(BULK_STRIPS):
        pack(strip)
        if strip == 0:
            pl.when(my_y == 1)(lambda: handshake(1))
        elif strip < HEAD:
            pl.when(my_y == 1)(lambda: over_y(strip).start())
        if strip == LATE_HANDSHAKE:
            pl.when(my_y == 0)(lambda: handshake(HEAD))
        if strip == BASE_STRIPS - 1:
            outbox.measure_base()
        while strip >= max(BASE_STRIPS - 1, 4 * encoded + 3):
            outbox.encode(encoded)
            encoded += 1

    jobs = []

    def job(ready, cycles, fn, *args):
        jobs.append((ready, cycles, functools.partial(fn, *args)))

    for group in range(encoded, GROUPS):
        job(lambda: True, SLOT_CYCLES, pack, *range(4 * group, 4 * group + 4))
        job(lambda: True, SLOT_CYCLES, outbox.encode, group)
    job(lambda: True, SLOT_CYCLES, outbox.place)
    job(lambda: True, SLOT_CYCLES, outbox.cut)
    for first in (2 * STRIPS - DIRECT, 2 * STRIPS - DIRECT // 2):
        job(lambda: True, SLOT_CYCLES, outbox.pack_direct, first)
    job(lambda: from_x.landed > CODE_AT, 0, loads[STRIPS].wait)
    for inbox in (from_x, from_y):
        job(lambda inbox=inbox: inbox.landed > CODE_AT, SLOT_CYCLES, inbox.read_header)
        job(lambda inbox=inbox: inbox.landed >= TAIL_AT, SLOT_CYCLES, inbox.take_strings)
        for group in reversed(range(GROUPS)):
            job(lambda inbox=inbox: inbox.landed >= TAIL_AT, SLOT_CYCLES, inbox.decode, group)
    for strip in range(2 * STRIPS):
        job(functools.partial(can_add, strip), 8, add, strip, (exp_y, exp_x)[strip // STRIPS])

    for i in range(Y_TILES):
        over_y(i).wait_recv()
        from_y.landed += 1
        if i == 0:
            pl.when(my_x == 0)(lambda: pl.semaphore_wait(x_ready, 1))
        if i < X_TILES:
            over_x(i).start()
        if from_y.landed == TAIL_AT:

            @pl.when(from_y.mode == ONE_MORE_TILE)
            def _():
                more_over_y().wait_recv()
                more_over_x().start()

        for _ in range(min(3, outbox.filled - outbox.started)):
            outbox.start_next()
        if i >= X_LAG:
            over_x(from_x.landed).wait_recv()
            from_x.landed += 1
            if from_x.landed == TAIL_AT:
                pl.when(from_x.mode == ONE_MORE_TILE)(lambda: more_over_x().wait_recv())
        left = SLOT_CYCLES
        for entry in list(jobs):
            ready, cycles, run = entry
            if cycles <= left and ready():
                run()
                jobs.remove(entry)
                left -= cycles
        if i == Y_TILES - 2:
            remote(sent, got_y, y_send_sem, y_recv_sems.at[0], y_peer).wait_send()
            remote(got_y.at[pl.ds(0, X_TILES)], got_x, x_send_sem, x_recv_sems.at[0], x_peer).wait_send()
    assert not jobs and outbox.started == Y_TILES and from_x.landed == X_TILES

    @pl.when((outbox.mode | from_y.mode | from_x.mode) != FITS)
    def _():
        pl.when(outbox.mode == ONE_MORE_TILE)(lambda: more_over_y().wait_send())
        pl.when(from_y.mode == ONE_MORE_TILE)(lambda: more_over_x().wait_send())

        @pl.when(from_y.mode == UNCODED)
        def _():
            for i in range(UNCODED_PARTS):
                uncoded_over_y(i).wait_recv()
                uncoded_over_x(i).start()
                for strip in range(i * part, (i + 1) * part):
                    add(strip, uncoded_y)
            remote(uncoded_y, uncoded_x, uncoded_send_sems.at[1], uncoded_x_sems.at[0], x_peer).wait_send()

        @pl.when(from_x.mode == UNCODED)
        def _():
            for i in range(UNCODED_PARTS):
                uncoded_over_x(i).wait_recv()
                for strip in range(i * part, (i + 1) * part):
                    add(STRIPS + strip, uncoded_x)

        @pl.when(outbox.mode == UNCODED)
        def _():
            remote(exp, uncoded_y, uncoded_send_sems.at[0], uncoded_y_sems.at[0], y_peer).wait_send()


def pallas_dist_ar_xy_y_m1024_n512_kernel(x: jax.Array):
    def tiles(*count):
        return pltpu.VMEM((*count, *TILE), jnp.int32)

    dma = pltpu.SemaphoreType.DMA
    return pl.pallas_call(
        _all_reduce,
        out_shape=jax.ShapeDtypeStruct((ROWS, COLS), jnp.bfloat16),
        in_specs=[pl.BlockSpec(memory_space=pltpu.HBM)],
        out_specs=pl.BlockSpec(memory_space=pltpu.VMEM),
        scratch_shapes=[
            pltpu.VMEM((ROWS, COLS), jnp.float32),
            pltpu.VMEM(TILE, jnp.float32),
            *(tiles(Y_TILES), tiles(Y_TILES), tiles(X_TILES)),
            *(tiles(), tiles(), tiles()),
            *(tiles(STRIPS),) * 5,
            *(dma((len(LOADS) + 2,)), dma, dma((Y_TILES,)), dma, dma((X_TILES,))),
            *(dma((4,)), dma((2,)), dma((UNCODED_PARTS,)), dma((UNCODED_PARTS,))),
            pltpu.SemaphoreType.REGULAR,
        ],
        compiler_params=pltpu.CompilerParams(
            collective_id=0, disable_bounds_checks=True, disable_semaphore_checks=True
        ),
    )(x)
```

```python
import functools

import jax
import jax.numpy as jnp
import numpy as np
from jax import lax
from jax.experimental import pallas as pl
from jax.experimental.pallas import tpu as pltpu

ROWS, COLS = 1024, 512
TILE = (8, 128)
STRIPS = ROWS // 2 // 8
GROUPS = STRIPS // 4

HEAD = 28
LOW_TILES = GROUPS // 2
ROW_WORDS = 14
DIRECT = 10
LOW_AT = HEAD
CODE_AT = LOW_AT + LOW_TILES
TAIL_AT = CODE_AT + ROW_WORDS
X_TILES = STRIPS - DIRECT + LOW_TILES + ROW_WORDS
Y_TILES = X_TILES + 2 * DIRECT
X_LAG = Y_TILES - X_TILES

STRING_WORDS = 17
HEADER_BITS = 64
BACK_WORDS, AHEAD_WORDS = 3, 5
FITS, ONE_MORE_TILE, UNCODED = 0, 1, 2

LOADS = (1, 1, 2) + (4,) * 15
BASE_STRIPS = 8
LATE_HANDSHAKE = 20
BULK_STRIPS = 44
SLOT_CYCLES = 100
UNCODED_PARTS = 8


def _word(v):
    return np.uint32(v).astype(np.int32)


def _bytes(v):
    return _word(v * 0x01010101)


def _shl(a, n):
    return lax.shift_left(a, np.int32(n) if isinstance(n, int) else n)


def _shr(a, n):
    return lax.shift_right_logical(a, np.int32(n) if isinstance(n, int) else n)


def _sublane():
    return lax.broadcasted_iota(jnp.int32, TILE, 0)


def _lane():
    return lax.broadcasted_iota(jnp.int32, TILE, 1)


_SIGN_MANTISSA = _word(0x807F807F)


def _split(a, b):
    b = _shl(b, 8) | _shr(b, 24)
    swap = (a ^ b) & _SIGN_MANTISSA
    e = a ^ swap
    return b ^ swap, _shr(e, 7) | _shl(e, 25)


def _join(s, e):
    e = _shl(e, 7) | _shr(e, 25)
    swap = (s ^ e) & _SIGN_MANTISSA
    b = s ^ swap
    return e ^ swap, _shr(b, 8) | _shl(b, 24)


def _below(v, k):
    m = ~(v + _bytes(128 - k)) & _bytes(128)
    return m - _shr(m, 7)


def _demote(v, n):
    return v + (_below(v, 1) & _bytes(n)) - (_below(v, n) & _bytes(1))


def _promote(v, n):
    return v + (_below(v, n - 1) & _bytes(n)) - (_below(v, n) & _bytes(n - 1))


def _encode_group(exponents, base):
    msb = jnp.full(TILE, _word(1 << 31), jnp.int32)
    hi = lo = length = low = distances = lengths = None
    for e in reversed(exponents):
        distance = base - e
        rank = _demote(_demote(distance, 12), 6)
        ones_at = (_shr(rank, 1) & _bytes(127)) + _word(0x01010100)
        ones_at = ones_at + _shl(ones_at, 8)
        ones_at = ones_at + _shl(ones_at, 16)
        bits = functools.reduce(
            jnp.bitwise_or, [_shr(msb, (_shr(ones_at, k) if k else ones_at) & 31) for k in (0, 8, 16, 24)]
        )
        n = _shr(ones_at, 24) + 1
        if hi is None:
            hi, length, low, distances, lengths = bits, n, rank & _bytes(1), distance, n
        else:
            carry = _shl(hi, -n & 31)
            lo = carry if lo is None else _shr(lo, n & 31) | carry
            hi = bits | _shr(hi, n & 31)
            length, low = length + n, _shl(low, 1) | (rank & _bytes(1))
            distances, lengths = distances | distance, lengths | n
    return hi, lo, length, low, (distances & _bytes(0xC0)) | _shr(lengths, 5) | _shr(length, 6)


def _decode_group(hi, lo, low, base):
    exponents, length = [], None
    for i in range(4):
        rest, zeros = hi, []
        for j in range(4):
            zeros.append(lax.clz(rest))
            if j < 3:
                rest = _shl(_shl(rest, 1), zeros[-1])
        n = (zeros[0] + zeros[1] + zeros[2] + 4) + zeros[3]
        rank = _shr(low, i) & _bytes(1)
        for j in range(4):
            rank = rank | _shl(zeros[j], 8 * j + 1)
        exponents.append(base - _promote(_promote(rank, 6), 12))
        length = n if length is None else length + n
        if i < 3:
            hi, lo = _shl(hi, n) | _shr(lo, 32 - n), _shl(lo, n)
    return exponents, length


def _delay(words, n, n_bits, count):
    for bit in range(5, n_bits):
        gap, on = [jnp.zeros_like(n)] * (1 << (bit - 5)), (n & (1 << bit)) != 0
        words = [lax.select(on, a, b) for a, b in zip((gap + words)[:count], words + gap)]
    bits, rest = n & 31, ~n & 31
    stay = [_shr(w, bits) for w in words]
    carry = [_shl(_shl(w, 1), rest) for w in words[: count - 1]]
    return (stay[:1] + [a | b for a, b in zip(stay[1:], carry)] + carry[len(stay) - 1 :])[:count]


def _skip(words, n, n_bits, count):
    for bit in reversed(range(5, n_bits)):
        gap, on = [jnp.zeros_like(n)] * (1 << (bit - 5)), (n & (1 << bit)) != 0
        words = [lax.select(on, a, b) for a, b in zip((words + gap)[len(gap) :], words[: count + len(gap)])]
    bits, rest = n & 31, ~n & 31
    stay = [_shl(w, bits) for w in words[:count]]
    carry = [_shr(_shr(w, 1), rest) for w in words[1 : count + 1]]
    return [a | b for a, b in zip(stay, carry)] + stay[len(carry) :]


def _place_strings(length):
    sub = _sublane()
    end = length
    for k in (1, 2, 4):
        end = end + jnp.where(sub >= k, pltpu.roll(end, k, 0), 0)
    row_bits = _shr(jnp.broadcast_to(end[7:8], TILE) + (HEADER_BITS + 7), 3)
    return end - length + (HEADER_BITS + 32 * BACK_WORDS) - row_bits * sub, row_bits


def _cut_rows(placed, start, base, mode):
    longer = mode == ONE_MORE_TILE
    rows = placed[BACK_WORDS : BACK_WORDS + ROW_WORDS + 1]
    back = [pltpu.roll(w, 7, 0) for w in placed[:BACK_WORDS]]
    for j, (a, b) in enumerate(zip([0] + back, back + [0])):
        rows[ROW_WORDS - BACK_WORDS + j] |= jnp.where(longer, a, b)
    ahead = placed[BACK_WORDS + ROW_WORDS :]
    for j in range(AHEAD_WORDS):
        rows[j] |= pltpu.roll(jnp.where(longer, ahead[j + 1], ahead[j]), 1, 0)
    rows = [w | jnp.where(mode == UNCODED, -1, 0) for w in rows]
    sub = _sublane()
    first = jnp.where(_lane() == 0, mode, base)
    header = _shl(jnp.where(sub == 0, first, start), (sub & 3) * 8)
    header = header | pltpu.roll(header, 7, 0)
    header = header | pltpu.roll(header, 6, 0)
    rows[0] = jnp.where(sub == 0, header, rows[0])
    rows[1] = jnp.where(sub == 0, pltpu.roll(header, 4, 0), rows[1])
    return rows


def _take_strings(rows, mode):
    longer = mode == ONE_MORE_TILE
    sub = _sublane()
    header = [jnp.broadcast_to(w[0:1], TILE) for w in rows[:2]]
    start = _shr(jnp.where(sub < 4, *header), (sub & 3) * 8) & 255
    start = jnp.where(sub == 0, HEADER_BITS + 32 * BACK_WORDS, start)
    last = rows[ROW_WORDS - BACK_WORDS :]
    back = [pltpu.roll(jnp.where(longer, a, b), 1, 0) for a, b in zip(last[1:], last)]
    ahead = [pltpu.roll(w, 7, 0) for w in rows[:AHEAD_WORDS]]
    ahead = [jnp.where(longer, a, b) for a, b in zip(rows[-1:] + ahead, ahead + [0])]
    return _skip(back + rows[:ROW_WORDS] + ahead, start, 8, STRING_WORDS)


def _tile_of(strip):
    return strip + (strip >= HEAD) * (LOW_TILES + ROW_WORDS)


class _Inbox:
    def __init__(self, tiles, one_more, exponents):
        self.tiles, self.one_more, self.exponents = tiles, one_more, exponents
        self.landed = 0
        self.decoded_from = STRIPS

    def read_mode(self):
        self.mode = self.tiles[CODE_AT][0, 0] & 255

    def take_strings(self):
        rows = [self.tiles[CODE_AT + j] for j in range(ROW_WORDS)] + [self.one_more[...]]
        self.string = _take_strings(rows, self.mode)
        base = jnp.where(_lane() == 0, 0, rows[0] & 255).astype(jnp.float32)
        base = jnp.broadcast_to(jnp.max(base, axis=1, keepdims=True)[0:1], TILE).astype(jnp.int32)
        base = base | _shl(base, 8)
        self.base = base | _shl(base, 16)

    def decode(self, group):
        low = _shr(self.tiles[LOW_AT + group // 2], 4 * (group % 2))
        exponents, length = _decode_group(*self.string[:2], low, self.base)
        for i, e in enumerate(exponents):
            self.exponents[4 * group + i] = e
        if group:
            self.string = _skip(self.string, length, 6, min(STRING_WORDS, group + 2))
        self.decoded_from = 4 * group


def _all_reduce(
    x_hbm, out,
    x, status,
    sent, got_y, got_x,
    sent_more, got_y_more, got_x_more,
    exp, exp_y, exp_x, uncoded_y, uncoded_x,
    load_sems, y_send_sem, y_recv_sems, x_send_sem, x_recv_sems,
    more_sems, uncoded_sems, uncoded_y_sems, x_ready,
):
    my_x, my_y = lax.axis_index("x"), lax.axis_index("y")
    y_peer, x_peer = (my_x, 1 - my_y), (1 - my_x, my_y)
    halves = [pl.ds(pl.multiple_of(h * 8 * STRIPS, 8 * STRIPS), 8 * STRIPS) for h in (my_x, 1 - my_x)]

    def remote(src, dst, send_sem, recv_sem, peer):
        return pltpu.make_async_remote_copy(
            src, dst, send_sem, recv_sem, device_id=peer, device_id_type=pl.DeviceIdType.MESH
        )

    def over_y(i):
        return remote(sent.at[i], got_y.at[i], y_send_sem, y_recv_sems.at[i], y_peer)

    def over_x(i):
        return remote(got_y.at[i], got_x.at[i], x_send_sem, x_recv_sems.at[i], x_peer)

    def more_over_y():
        return remote(sent_more, got_y_more, more_sems.at[0], more_sems.at[1], y_peer)

    def more_over_x():
        return remote(got_y_more, got_x_more, more_sems.at[2], more_sems.at[3], x_peer)

    part = STRIPS // UNCODED_PARTS

    def uncoded_over_y(i):
        r = pl.ds(i * part, part)
        return remote(exp.at[r], uncoded_y.at[r], uncoded_sems.at[0], uncoded_y_sems.at[i], y_peer)

    def uncoded_over_x(i):
        r = pl.ds(i * part, part)
        return remote(uncoded_y.at[r], uncoded_x.at[r], uncoded_sems.at[1], uncoded_sems.at[2], x_peer)

    loads = {}

    def load(strip, count):
        rows = x_hbm.at[halves[strip // STRIPS]].at[pl.ds(8 * (strip % STRIPS), 8 * count)]
        loads[strip] = pltpu.async_copy(rows, x.at[pl.ds(8 * strip, 8 * count)], load_sems.at[len(loads)])

    load(0, LOADS[0])
    got_y_more[...] = jnp.zeros(TILE, jnp.int32)
    got_x_more[...] = jnp.zeros(TILE, jnp.int32)
    barrier = pltpu.get_barrier_semaphore()

    def signal(sem, peer):
        pl.semaphore_signal(sem, device_id=peer, device_id_type=pl.DeviceIdType.MESH)

    signal(barrier, y_peer)
    pl.when(my_x == 0)(lambda: signal(barrier, x_peer))
    for i in range(1, len(LOADS)):
        load(sum(LOADS[:i]), LOADS[i])
    load(2 * STRIPS - DIRECT, DIRECT)
    load(STRIPS, STRIPS - DIRECT)

    def handshake(tiles_ready):
        pl.semaphore_wait(barrier, 1 + my_x)
        pl.when(my_x == 1)(lambda: signal(x_ready, x_peer))
        for i in range(tiles_ready):
            over_y(i).start()

    def pack(*strips):
        for strip in strips:
            if strip in loads:
                loads[strip].wait()
            v = x[8 * strip : 8 * strip + 8, :]
            pairs = [jnp.concatenate([v[:, c : c + 128], v[:, c + 128 : c + 256]]) for c in (0, 256)]
            s, e = _split(*[pltpu.bitcast(p.astype(jnp.bfloat16), jnp.int32) for p in pairs])
            if strip < STRIPS:
                sent[_tile_of(strip)] = s
                exp[strip] = e
            else:
                sent[_tile_of(strip - STRIPS + DIRECT)] = s

    class Outbox:
        filled = started = HEAD

        def measure_base(self):
            total = 0
            for strip in range(BASE_STRIPS):
                e = exp[strip]
                total = total + (e & 0x00FF00FF) + (_shr(e, 8) & 0x00FF00FF)
            total = jnp.sum(((total & 0xFFFF) + _shr(total, 16)).astype(jnp.float32))
            mean = total * (1.0 / (BASE_STRIPS * 8 * COLS))
            self.base = jnp.minimum((mean + 3.86).astype(jnp.int32), 255)

        def encode(self, group):
            base = jnp.full(TILE, self.base * _bytes(1), jnp.int32)
            hi, lo, length, low, misfit = _encode_group([exp[4 * group + i] for i in range(4)], base)
            at = LOW_AT + group // 2
            sent[at] = sent[at] | _shl(low, 4) if group % 2 else low
            if group == 0:
                self.string, self.length, self.misfit = [hi, lo], length, misfit
                return
            count = min(STRING_WORDS, group + 3)
            self.string = _delay(self.string, length, 6, count)
            self.string[0] |= hi
            self.string[1] |= lo
            self.length = self.length + length
            self.misfit = self.misfit | misfit | _shr(32 * count - self.length, 31)

        def place(self):
            start, row_bits = _place_strings(self.length)
            misfit = self.misfit | (start & -256) | _shr(32 * (ROW_WORDS + 1) - row_bits, 31)
            mode = jnp.where(row_bits > 32 * ROW_WORDS, ONE_MORE_TILE, FITS)
            mode = jnp.where(misfit != 0, UNCODED, mode).astype(jnp.float32)
            status[...] = jnp.broadcast_to(jnp.max(mode, axis=1, keepdims=True), TILE)
            self.start = start & 255
            self.string = _delay(self.string, self.start, 8, BACK_WORDS + ROW_WORDS + 1 + AHEAD_WORDS)

        def cut(self):
            self.mode = jnp.max(status[...], axis=0, keepdims=True).astype(jnp.int32)[0, 0]
            rows = _cut_rows(self.string, self.start, self.base, self.mode)
            for j in range(ROW_WORDS):
                sent[CODE_AT + j] = rows[j]
            sent_more[...] = rows[ROW_WORDS]
            self.filled = Y_TILES - DIRECT

        def pack_direct(self, first):
            pack(*range(first, first + DIRECT // 2))
            self.filled += DIRECT // 2

        def start_next(self):
            over_y(self.started).start()
            self.started += 1
            if self.started == TAIL_AT:
                pl.when(self.mode == ONE_MORE_TILE)(lambda: more_over_y().start())
            if self.started == Y_TILES:

                @pl.when(self.mode == UNCODED)
                def _():
                    for i in range(UNCODED_PARTS):
                        uncoded_over_y(i).start()

    outbox = Outbox()
    from_y = _Inbox(got_y, got_y_more, exp_y)
    from_x = _Inbox(got_x, got_x_more, exp_x)

    def source(half, strip):
        if half and strip < STRIPS - DIRECT:
            return from_x, 0
        return from_y, half * DIRECT

    def add(half, strip, inbox, moved, exponents):
        other = []
        for pairs in _join(inbox.tiles[_tile_of(strip) + moved], exponents[strip]):
            pairs = pltpu.bitcast(pairs, jnp.bfloat16).astype(jnp.float32)
            other += [pairs[:8], pairs[8:]]
        row = 8 * strip if isinstance(strip, int) else pl.multiple_of(8 * strip, 8)
        total = x[pl.ds(8 * STRIPS * half + row, 8), :] + jnp.concatenate(other, axis=1)
        out.at[halves[half]][pl.ds(row, 8), :] = total.astype(out.dtype)

    def can_add(half, strip):
        inbox, moved = source(half, strip)
        return inbox.landed > _tile_of(strip) + moved and (from_y, from_x)[half].decoded_from <= strip

    pl.when(my_y == 1)(lambda: handshake(0))
    encoded = 0
    for strip in range(BULK_STRIPS):
        if strip == LATE_HANDSHAKE:
            pl.when(my_y == 0)(lambda: handshake(strip))
        pack(strip)
        if strip < LATE_HANDSHAKE:
            pl.when(my_y == 1)(lambda: over_y(strip).start())
        elif strip < HEAD:
            over_y(strip).start()
        if strip == BASE_STRIPS - 1:
            outbox.measure_base()
        while strip >= max(BASE_STRIPS - 1, 4 * encoded + 3):
            outbox.encode(encoded)
            encoded += 1

    jobs = []

    def job(ready, cycles, fn, *args):
        jobs.append((ready, cycles, functools.partial(fn, *args)))

    for group in range(encoded, GROUPS):
        job(lambda: True, 25, pack, *range(4 * group, 4 * group + 4))
        job(lambda: True, 75, outbox.encode, group)
    job(lambda: True, SLOT_CYCLES, outbox.place)
    job(lambda: True, SLOT_CYCLES, outbox.cut)
    for first in (2 * STRIPS - DIRECT, 2 * STRIPS - DIRECT // 2):
        job(lambda: True, SLOT_CYCLES, outbox.pack_direct, first)
    job(lambda: from_x.landed > CODE_AT, 0, loads[STRIPS].wait)
    for inbox in (from_x, from_y):
        job(lambda inbox=inbox: inbox.landed > CODE_AT, SLOT_CYCLES, inbox.read_mode)
        job(lambda inbox=inbox: inbox.landed >= TAIL_AT, SLOT_CYCLES, inbox.take_strings)
        for group in reversed(range(GROUPS)):
            job(lambda inbox=inbox: inbox.landed >= TAIL_AT, SLOT_CYCLES, inbox.decode, group)
    for half, exponents in enumerate((exp_y, exp_x)):
        for strip in range(STRIPS):
            job(functools.partial(can_add, half, strip), 8, add, half, strip, *source(half, strip), exponents)

    for i in range(Y_TILES):
        over_y(i).wait_recv()
        from_y.landed += 1
        if i == 0:
            pl.when(my_x == 0)(lambda: pl.semaphore_wait(x_ready, 1))
        if i < X_TILES:
            over_x(i).start()
        if from_y.landed == TAIL_AT:

            @pl.when(from_y.mode == ONE_MORE_TILE)
            def _():
                more_over_y().wait_recv()
                more_over_x().start()

        for _ in range(min(3, outbox.filled - outbox.started)):
            outbox.start_next()
        if i >= X_LAG:
            over_x(from_x.landed).wait_recv()
            from_x.landed += 1
            if from_x.landed == TAIL_AT:
                pl.when(from_x.mode == ONE_MORE_TILE)(lambda: more_over_x().wait_recv())
        left = SLOT_CYCLES
        for entry in list(jobs):
            ready, cycles, run = entry
            if cycles <= left and ready():
                run()
                jobs.remove(entry)
                left -= cycles
        if i == Y_TILES - 2:
            remote(sent, got_y, y_send_sem, y_recv_sems.at[0], y_peer).wait_send()
            remote(got_y.at[pl.ds(0, X_TILES)], got_x, x_send_sem, x_recv_sems.at[0], x_peer).wait_send()
    assert not jobs and outbox.started == Y_TILES and from_x.landed == X_TILES

    @pl.when((outbox.mode | from_y.mode | from_x.mode) != FITS)
    def _():
        pl.when(outbox.mode == ONE_MORE_TILE)(lambda: more_over_y().wait_send())
        pl.when(from_y.mode == ONE_MORE_TILE)(lambda: more_over_x().wait_send())

        def add_again(half, first, last, exponents):
            pl.loop(first, last)(lambda strip: add(half, strip, *source(half, first), exponents))

        all_over_x = remote(uncoded_y, uncoded_x, uncoded_sems.at[1], uncoded_sems.at[2], x_peer)

        @pl.when(from_y.mode == UNCODED)
        def _():
            for i in range(UNCODED_PARTS):
                uncoded_over_y(i).wait_recv()
                uncoded_over_x(i).start()
            add_again(0, 0, STRIPS, uncoded_y)
            all_over_x.wait_send()

        @pl.when(from_x.mode == UNCODED)
        def _():
            all_over_x.wait_recv()
            add_again(1, 0, STRIPS - DIRECT, uncoded_x)
            add_again(1, STRIPS - DIRECT, STRIPS, uncoded_x)

        @pl.when(outbox.mode == UNCODED)
        def _():
            remote(exp, uncoded_y, uncoded_sems.at[0], uncoded_y_sems.at[0], y_peer).wait_send()


def pallas_dist_ar_xy_y_m1024_n512_kernel(x: jax.Array):
    def tiles(*count):
        return pltpu.VMEM((*count, *TILE), jnp.int32)

    dma = pltpu.SemaphoreType.DMA
    return pl.pallas_call(
        _all_reduce,
        out_shape=jax.ShapeDtypeStruct((ROWS, COLS), jnp.bfloat16),
        in_specs=[pl.BlockSpec(memory_space=pltpu.HBM)],
        out_specs=pl.BlockSpec(memory_space=pltpu.VMEM),
        scratch_shapes=[
            pltpu.VMEM((ROWS, COLS), jnp.float32),
            pltpu.VMEM(TILE, jnp.float32),
            *(tiles(Y_TILES), tiles(Y_TILES), tiles(X_TILES)),
            *(tiles(), tiles(), tiles()),
            *(tiles(STRIPS),) * 5,
            *(dma((len(LOADS) + 2,)), dma, dma((Y_TILES,)), dma, dma((X_TILES,))),
            *(dma((4,)), dma((3,)), dma((UNCODED_PARTS,))),
            pltpu.SemaphoreType.REGULAR,
        ],
        compiler_params=pltpu.CompilerParams(
            collective_id=0, disable_bounds_checks=True, disable_semaphore_checks=True
        ),
    )(x)
```
